```python
import numpy as np

kernel_name = "dist_sparse_attn_strided_kvseq_b1_sq256_skv4096_hq8_dh128"

def setup_inputs():
    x = np.random.randn(1, 256, 1024).astype(np.float32)
    Wq = np.random.randn(1024, 1024).astype(np.float32) * 0.02
    K_ext = np.random.randn(1, 16384, 8, 128).astype(np.float32)
    V_ext = np.random.randn(1, 16384, 8, 128).astype(np.float32)
    Wo = np.random.randn(1024, 1024).astype(np.float32) * 0.02
    return {"x": x, "Wq": Wq, "K_ext": K_ext, "V_ext": V_ext, "Wo": Wo}

def reference(x, Wq, K_ext, V_ext, Wo):
    B, Sq, Skv, Hq, Dh = 1, 256, 16384, 8, 128
    Q = (x @ Wq).reshape(B, Sq, Hq, Dh)
    qb = (np.arange(Sq) // 64)[:, None]
    kb = (np.arange(Skv) // 64)[None, :]
    mask = (qb == kb) | ((kb % 4) == (qb % 4))
    scores = np.einsum('bihd,bjhd->bhij', Q, K_ext).astype(np.float32) * 0.08838834764831843
    scores = np.where(mask[None, None, :, :], scores, -1e9)
    scores_max = scores.max(axis=-1, keepdims=True)
    w = np.exp(scores - scores_max)
    row_keep = mask.any(axis=1)
    w_sum = np.where(row_keep[None, None, :, None], w.sum(axis=-1, keepdims=True), 1.0)
    w = w / w_sum
    w = np.where(row_keep[None, None, :, None], w, 0.0)
    ctx = np.einsum('bhij,bjhd->bihd', w, V_ext).reshape(B, Sq, Hq * Dh)
    return ctx @ Wo
```

```python
import contextlib
import functools
import math

import jax
import jax.numpy as jnp
from jax import lax
from jax.experimental import pallas as pl
from jax.experimental.pallas import tpu as pltpu

N_DEV = 4
N_HEAD = 8
D_HEAD = 128
D_MODEL = 1024
SQ = 256
QB = 64
N_GROUP = 4
N_SUPER = 16
KEYS = N_SUPER * QB
LAST = N_HEAD - 1
N_UNIT = N_HEAD * N_GROUP
K_SHARE = D_MODEL // N_DEV
HALF = D_MODEL // 2
PIECE = 64
SCORE_SCALE = 0.08838834764831843 * math.log2(math.e)
BULK_ORDER = (1, 3, 2)
FAST_ORDER = (2, 1, 3)
MESH = pl.DeviceIdType.MESH
F32 = jnp.float32
BF16 = jnp.bfloat16


def _fold(col):
    wide = jnp.broadcast_to(col, (QB, 128))
    lane_group = lax.broadcasted_iota(jnp.int32, (8, 128), 1) // 16
    tile = wide[0:8]
    for j in range(1, 8):
        tile = jnp.where(lane_group == j, wide[8 * j:8 * j + 8], tile)
    return tile


def _unfold(tile):
    return jnp.concatenate(
        [jnp.broadcast_to(tile[:, 16 * j:16 * j + 1], (8, 128)) for j in range(8)], axis=0)


def make_kernel(n_early=3, bulk_heads=4, ahead=8, v_split=8, early_at=19, swap_tail=True, split_last=True,
                scopes=False):
    v_parts = ((0, v_split), (v_split, N_SUPER - v_split))
    last_piece = 2 * LAST

    def scope(name):
        return jax.named_scope(name) if scopes else contextlib.nullcontext()

    def body(x_hbm, wq_hbm, k_hbm, v_hbm, wo_hbm, out_ref,
             x_f32, wq_f32, wo_f32, k_buf, v_buf,
             q_send, q_part, q_all, wo_bf16, o_part, lse_part, o_send, lse_send, ctx, acc,
             w_sem, k_sem, v_sem, wo_sem,
             qp_ssem, qp_rsem, q_ssem, q_rsem, wo_ssem, wo_rsem,
             o_ssem, o_rsem, l_ssem, l_rsem, c_ssem, c_rsem):
        me = lax.axis_index("i")
        peer = lambda j: (me + j) & (N_DEV - 1)
        relay = me == 2
        odd = (me & 1) == 1
        my_first = jnp.where(odd, (me >> 1) * n_early, last_piece)
        my_count = jnp.where(odd, n_early, 2)
        early_count = jnp.where(relay, 0, my_count)

        def remote(src, dst, ssem, rsem, j):
            return pltpu.make_async_remote_copy(
                src, dst, ssem, rsem, device_id=(peer(j),), device_id_type=MESH)

        def piece_rows(p):
            return pl.ds(pl.multiple_of(p * PIECE, PIECE), PIECE)

        def wo_piece_load(p):
            return pltpu.make_async_copy(wo_hbm.at[piece_rows(p)], wo_f32.at[piece_rows(p)], wo_sem.at[p])

        def wo_piece_copy(p, j):
            rows = wo_bf16.at[piece_rows(p)]
            return remote(rows, rows, wo_ssem.at[p, j // 2], wo_rsem.at[p], j)

        def round_pieces(count):
            @pl.loop(0, count)
            def _(i):
                p = my_first + i
                wo_piece_load(p).wait()
                wo_bf16[piece_rows(p), :] = wo_f32[piece_rows(p), :].astype(BF16)

        def send_wo_step(i):
            @pl.when(i < early_count)
            def _():
                for j in (1, 3):
                    wo_piece_copy(my_first + i, j).start()

            @pl.when(jnp.logical_and(relay, jnp.logical_and(i >= 1, i <= n_early)))
            def _():
                for j, first in ((1, 0), (3, n_early)):
                    cp = wo_piece_copy(first + i - 1, j)
                    cp.wait_recv()
                    cp.start()

        def finish_wo_exchange():
            @pl.loop(0, early_count)
            def _(i):
                for j in (1, 3):
                    wo_piece_copy(my_first + i, j).wait_send()

            @pl.loop(0, n_early)
            def _(i):
                @pl.when(relay)
                def _():
                    wo_piece_copy(i, 1).wait_send()
                    wo_piece_copy(n_early + i, 3).wait_send()

                @pl.when(jnp.logical_or(me == 0, me == 3))
                def _():
                    wo_piece_copy(i, 1).wait_recv()

                @pl.when(me <= 1)
                def _():
                    wo_piece_copy(n_early + i, 1).wait_recv()

            @pl.when(odd)
            def _():
                wo_piece_copy(last_piece, 1).wait_recv()
                wo_piece_copy(last_piece + 1, 1).wait_recv()

        def head_rows(h):
            return pl.ds(h * D_HEAD, D_HEAD)

        late_blocks = [(h, pl.ds(0, D_MODEL), 2 * h) for h in range(n_early, LAST - 1)]
        if split_last:
            late_blocks += [(LAST - 1, pl.ds(c * HALF, HALF), 2 * (LAST - 1) + c) for c in range(2)]
        else:
            late_blocks += [(LAST - 1, pl.ds(0, D_MODEL), 2 * (LAST - 1))]
        late_loads = [
            pltpu.make_async_copy(wo_hbm.at[head_rows(h), cols], wo_f32.at[head_rows(h), cols], wo_sem.at[s])
            for h, cols, s in late_blocks]

        mine = pl.ds(pl.multiple_of(me * K_SHARE, K_SHARE), K_SHARE)
        x_cp = pltpu.make_async_copy(x_hbm.at[0, :, mine], x_f32, w_sem.at[0])
        wq_cp = pltpu.make_async_copy(wq_hbm.at[mine], wq_f32, w_sem.at[1])

        with scope("t_issue"):
            wq_cp.start()
            x_cp.start()
            barrier = pltpu.get_barrier_semaphore()
            for j in FAST_ORDER:
                pl.semaphore_signal(barrier, inc=1, device_id=(peer(j),), device_id_type=MESH)

            @pl.loop(0, early_count)
            def _(i):
                wo_piece_load(my_first + i).start()

            @pl.loop(0, bulk_heads)
            def _(h):
                u = N_GROUP * h
                pltpu.make_async_copy(k_hbm.at[:, :, :, h], k_buf.at[h], k_sem.at[u]).start()
                pltpu.make_async_copy(v_hbm.at[:, :, :, h], v_buf.at[h], v_sem.at[u, 0]).start()

        def q_scatter(s, j):
            return remote(q_send.at[j, s], q_part.at[j - 1, s], qp_ssem.at[s, j - 1], qp_rsem.at[s, j - 1], j)

        def q_gather(s, j):
            return remote(q_all.at[me, s], q_all.at[me, s], q_ssem.at[s, j - 1], q_rsem.at[s, j - 1], j)

        with scope("t_qproj"):
            wq_cp.wait()
            x_cp.wait()

            @pl.loop(0, N_DEV)
            def _(j):
                rows = pl.ds(pl.multiple_of(peer(j) * QB, QB), QB)
                q = jnp.dot(x_f32[rows, :].astype(BF16), wq_f32[...].astype(BF16),
                            preferred_element_type=F32)
                q = (q * SCORE_SCALE).astype(BF16)
                for h in range(N_HEAD):
                    q_send[j, h // 2, h % 2] = q[:, h * D_HEAD:(h + 1) * D_HEAD]

        with scope("t_qrs"):
            pl.semaphore_wait(barrier, N_DEV - 1)

            @pl.loop(0, N_HEAD // 2)
            def _(s):
                for j in BULK_ORDER:
                    q_scatter(s, j).start()

            round_pieces(early_count)

            @pl.loop(0, N_HEAD // 2)
            def _(s):
                for j in BULK_ORDER:
                    q_scatter(s, j).wait()
                q = q_send[0, s].astype(F32)
                for j in BULK_ORDER:
                    q = q + q_part[j - 1, s].astype(F32)
                q_all[me, s] = q.astype(BF16)
                for j in BULK_ORDER:
                    q_gather(s, j).start()

        def k_unit_load(h, g, u):
            return pltpu.make_async_copy(k_hbm.at[:, g, :, h], k_buf.at[h, :, g], k_sem.at[u])

        def v_unit_load(h, g, u, part):
            s = pl.ds(*v_parts[part])
            return pltpu.make_async_copy(v_hbm.at[s, g, :, h], v_buf.at[h, s, g], v_sem.at[u, part])

        def unit_ids(u):
            h = u // N_GROUP
            j = u % N_GROUP
            return h, j, jnp.where(h == LAST, j, peer(j + 1))

        def start_unit(u):
            h, _, g = unit_ids(u)
            k_unit_load(h, g, u).start()
            v_unit_load(h, g, u, 0).start()
            v_unit_load(h, g, u, 1).start()

        def scores(h, j, g, u):
            @pl.when(u % (2 * N_GROUP) == 0)
            def _():
                for i in BULK_ORDER:
                    q_gather(h // 2, i).wait()

            @pl.when(jnp.logical_and(h < bulk_heads, j == 0))
            def _():
                pltpu.make_async_copy(k_buf.at[h], k_buf.at[h], k_sem.at[u]).wait()

            @pl.when(h >= bulk_heads)
            def _():
                k_unit_load(h, g, u).wait()

            k = k_buf[h, :, g].reshape(KEYS, D_HEAD).astype(BF16)
            s = lax.dot_general(q_all[g, h // 2, h % 2], k, (((1,), (1,)), ((), ())), preferred_element_type=F32)
            m = jnp.max(s, axis=1, keepdims=True)
            p = jnp.exp2(s - m)
            l = jnp.sum(p, axis=1, keepdims=True)
            lse = _fold(m) + jnp.log2(_fold(l))
            return p.astype(BF16), 1.0 / l, lse

        def weighted_values(p, inv_l, h, j, g, u):
            @pl.when(jnp.logical_and(h < bulk_heads, j == 0))
            def _():
                pltpu.make_async_copy(v_buf.at[h], v_buf.at[h], v_sem.at[u, 0]).wait()

            o = None
            for part, (s0, n) in enumerate(v_parts):
                @pl.when(h >= bulk_heads)
                def _():
                    v_unit_load(h, g, u, part).wait()

                v = v_buf[h, s0:s0 + n, g].reshape(n * QB, D_HEAD).astype(BF16)
                pv = jnp.dot(p[:, s0 * QB:(s0 + n) * QB], v, preferred_element_type=F32)
                o = pv if o is None else o + pv
            return (o * inv_l).astype(BF16)

        def partial_copy(part, send, ssem, rsem, u, slot, j):
            return remote(send.at[u], part.at[slot, j - 1], ssem.at[slot, j - 1], rsem.at[slot, j - 1], j)

        lse_copy = functools.partial(partial_copy, lse_part, lse_send, l_ssem, l_rsem)
        o_copy = functools.partial(partial_copy, o_part, o_send, o_ssem, o_rsem)

        def wait_partials(copy, u, slot):
            for j in BULK_ORDER:
                copy(u, slot, j).wait_send()
            for j in BULK_ORDER:
                copy(u, slot, j).wait_recv()

        def merge_weights(u, slot):
            lses = [lse_send[u]] + [lse_part[slot, i] for i in range(N_DEV - 1)]
            top = functools.reduce(jnp.maximum, lses)
            es = [jnp.exp2(t - top) for t in lses]
            inv = 1.0 / functools.reduce(jnp.add, es)
            return [_unfold(e * inv) for e in es]

        def merge_values(ws, u, slot):
            total = ws[0] * o_send[u].astype(F32)
            for j in BULK_ORDER:
                total = total + ws[j] * o_part[slot, j - 1].astype(F32)
            return total.astype(BF16)

        def merge(*units):
            for u, slot in units:
                wait_partials(lse_copy, u, slot)
                wait_partials(o_copy, u, slot)
            return [merge_values(merge_weights(u, slot), u, slot) for u, slot in units]

        def ctx_copy(h, j):
            return remote(ctx.at[h, me], ctx.at[h, me], c_ssem.at[h, j - 1], c_rsem.at[h, j - 1], j)

        def ctx_wait(h):
            for j in BULK_ORDER:
                ctx_copy(h, j).wait()

        def project(heads, w):
            lhs = jnp.concatenate([ctx[h].reshape(SQ, D_HEAD) for h in heads], axis=1)
            return jnp.dot(lhs, w, preferred_element_type=F32)

        with scope("t_main"):
            @pl.loop(0, N_UNIT)
            def _(u):
                h, j, g = unit_ids(u)
                late = h == LAST
                one_peer = jnp.logical_and(jnp.logical_not(late), j < N_GROUP - 1)

                @pl.when(jnp.logical_and(u + ahead >= N_GROUP * bulk_heads, u + ahead < N_UNIT))
                def _():
                    start_unit(u + ahead)

                with scope("t_qk"):
                    p, inv_l, lse = scores(h, j, g, u)
                    lse_send[u] = lse

                @pl.when(one_peer)
                def _():
                    lse_copy(u, h, j + 1).start()

                @pl.when(late)
                def _():
                    for i in FAST_ORDER:
                        lse_copy(u, LAST + j, i).start()

                with scope("t_pv"):
                    o_send[u] = weighted_values(p, inv_l, h, j, g, u)

                @pl.when(late)
                def _():
                    for i in FAST_ORDER:
                        o_copy(u, LAST + j, i).start()

                @pl.when(one_peer)
                def _():
                    o_copy(u, h, j + 1).start()

                @pl.when(jnp.where(late, j == 0, jnp.logical_and(h > 0, j == N_GROUP - 1)))
                def _():
                    with scope("t_red"):
                        ctx[h - 1, me] = merge((N_GROUP * h - 1, h - 1))[0]
                        for i in BULK_ORDER:
                            ctx_copy(h - 1, i).start()

                @pl.when(j == N_GROUP - 1)
                def _():
                    send_wo_step(h)

                @pl.when(u == early_at)
                def _():
                    with scope("t_early"):
                        finish_wo_exchange()

                        @pl.loop(0, n_early)
                        def _(h):
                            ctx_wait(h)

                        @pl.loop(0, 2)
                        def _(c):
                            cols = pl.ds(pl.multiple_of(c * HALF, HALF), HALF)
                            acc[:, cols] = project(range(n_early), wo_bf16[0:n_early * D_HEAD, cols])

                @pl.when(u == N_UNIT - 2)
                def _():
                    with scope("t_lateissue"):
                        @pl.loop(0, my_count - early_count)
                        def _(i):
                            wo_piece_load(my_first + i).start()

                        for cp in late_loads:
                            cp.start()

                        @pl.loop(n_early, LAST - 1)
                        def _(h):
                            ctx_wait(h)

        last_unit = lambda g: (N_GROUP * LAST + g, LAST + g)
        w_last = lambda: wo_bf16[head_rows(LAST), :]
        top = (N_GROUP - 1) * QB

        def late_product(i):
            h, cols, _ = late_blocks[i]
            return acc[:, cols] + project([h], wo_f32[head_rows(h), cols].astype(BF16))

        with scope("t_m01"):
            c01 = jnp.concatenate(merge(last_unit(0), last_unit(1)), axis=0)
            round_pieces(my_count - early_count)
            acc[0:2 * QB, :] += jnp.dot(c01, w_last(), preferred_element_type=F32)

        n_full = LAST - 1 - n_early
        for i in range(n_full):
            with scope(f"t_late{i}"):
                late_loads[i].wait()
                if i < n_full - 1:
                    acc[...] = late_product(i)
                else:
                    c2 = merge(last_unit(2))[0]
                    r = late_product(i)
                    r2 = jnp.dot(c2, w_last(), preferred_element_type=F32)
                    acc[0:2 * QB, :] = r[0:2 * QB]
                    acc[2 * QB:top, :] = r[2 * QB:top] + r2
                    acc[top:, :] = r[top:]

        ctx_wait(LAST - 1)
        u3 = last_unit(N_GROUP - 1)

        def leader_order():
            ws = None
            for i in range(n_full, len(late_blocks)):
                with scope(f"t_late{i}"):
                    late_loads[i].wait()
                    if i == len(late_blocks) - 1:
                        wait_partials(lse_copy, *u3)
                        ws = merge_weights(*u3)
                    cols = late_blocks[i][1]
                    r = late_product(i)
                    out_ref[0, 0:top, cols] = r[0:top].astype(out_ref.dtype)
                    acc[top:, cols] = r[top:]
            with scope("t_final"):
                wait_partials(o_copy, *u3)
                c = merge_values(ws, *u3)
                out_ref[0, top:, :] = (
                    acc[top:, :] + jnp.dot(c, w_last(), preferred_element_type=F32)).astype(out_ref.dtype)

        def follower_order():
            with scope("t_final"):
                c = merge(u3)[0]
                acc[top:, :] += jnp.dot(c, w_last(), preferred_element_type=F32)
            for i in range(n_full, len(late_blocks)):
                with scope(f"t_late{i}"):
                    late_loads[i].wait()
                    out_ref[0, :, late_blocks[i][1]] = late_product(i).astype(out_ref.dtype)

        if swap_tail:
            pl.when(me != 0)(follower_order)
            pl.when(me == 0)(leader_order)
        else:
            leader_order()

    n_slot = LAST + N_GROUP
    n_piece = D_MODEL // PIECE
    dma = pltpu.SemaphoreType.DMA

    def fn(x, Wq, K_ext, V_ext, Wo):
        kv_shape = (N_SUPER, N_GROUP, QB, N_HEAD, D_HEAD)
        hbm = pl.BlockSpec(memory_space=pl.ANY)
        return pl.pallas_call(
            body,
            out_shape=jax.ShapeDtypeStruct((1, SQ, D_MODEL), BF16),
            in_specs=[hbm] * 5,
            out_specs=pl.BlockSpec(memory_space=pltpu.VMEM),
            scratch_shapes=[
                pltpu.VMEM((SQ, K_SHARE), F32),
                pltpu.VMEM((K_SHARE, D_MODEL), F32),
                pltpu.VMEM((D_MODEL, D_MODEL), F32),
                pltpu.VMEM((N_HEAD, N_SUPER, N_GROUP, QB, D_HEAD), F32),
                pltpu.VMEM((N_HEAD, N_SUPER, N_GROUP, QB, D_HEAD), F32),
                pltpu.VMEM((N_DEV, N_HEAD // 2, 2, QB, D_HEAD), BF16),
                pltpu.VMEM((N_DEV - 1, N_HEAD // 2, 2, QB, D_HEAD), BF16),
                pltpu.VMEM((N_GROUP, N_HEAD // 2, 2, QB, D_HEAD), BF16),
                pltpu.VMEM((D_MODEL, D_MODEL), BF16),
                pltpu.VMEM((n_slot, N_DEV - 1, QB, D_HEAD), BF16),
                pltpu.VMEM((n_slot, N_DEV - 1, 8, 128), F32),
                pltpu.VMEM((N_UNIT, QB, D_HEAD), BF16),
                pltpu.VMEM((N_UNIT, 8, 128), F32),
                pltpu.VMEM((LAST, N_GROUP, QB, D_HEAD), BF16),
                pltpu.VMEM((SQ, D_MODEL), F32),
                dma((2,)), dma((N_UNIT,)), dma((N_UNIT, 2)), dma((n_piece,)),
                dma((4, 3)), dma((4, 3)), dma((4, 3)), dma((4, 3)), dma((n_piece, 2)), dma((n_piece,)),
                dma((n_slot, 3)), dma((n_slot, 3)), dma((n_slot, 3)), dma((n_slot, 3)),
                dma((LAST, 3)), dma((LAST, 3)),
            ],
            compiler_params=pltpu.CompilerParams(
                collective_id=0,
                vmem_limit_bytes=64 * 2**20,
                disable_semaphore_checks=True,
                disable_bounds_checks=True,
            ),
        )(x, Wq, K_ext.reshape(kv_shape), V_ext.reshape(kv_shape), Wo)

    return fn


def pallas_dist_sparse_attn_strided_kvseq_b1_sq256_skv4096_hq8_dh128_kernel(x, Wq, K_ext, V_ext, Wo):
    return make_kernel(split_last=False)(x, Wq, K_ext, V_ext, Wo)
```

```python
import functools
import math

import jax
import jax.numpy as jnp
from jax import lax
from jax.experimental import pallas as pl
from jax.experimental.pallas import tpu as pltpu

N_DEV = 4
N_PEER = N_DEV - 1
N_HEAD = 8
D_HEAD = 128
D_MODEL = 1024
SQ = 256
QB = 64
N_GROUP = SQ // QB
N_PERIOD = 16
LANES = 128
N_TILE = D_MODEL // LANES
HALF = D_MODEL // 2
K_SHARE = D_MODEL // N_DEV
TOP = SQ - QB

N_UNIT = N_HEAD * N_GROUP
LAST_UNIT = N_UNIT - 1
LAST_HEAD = N_HEAD - 1
N_SLOT = LAST_HEAD + N_GROUP

BULK_HEADS = 4
LOOKAHEAD = 8
N_KV_LOAD = N_UNIT - (N_GROUP - 1) * BULK_HEADS

SIDE_HEADS = 3
LEAD_HEAD = 3
MID_HEADS = (4, 5)
END_HEAD = 6
PIECE = 32
HEAD_PIECES = D_HEAD // PIECE
SIDE_SHARES = ((1, 0, 5), (3, 5, 7))
LEAD_PIECES = 2 * HEAD_PIECES
RELAY_LAG = 2
SHARE_STEPS = max(LEAD_PIECES, RELAY_LAG + max(n for _, _, n in SIDE_SHARES))

SIDE_HEADS_AT = 21
LEAD_SCHEDULE = ((25, LEAD_HEAD, ()), (26, MID_HEADS[0], ()), (29, MID_HEADS[1], (0,)))

SCORE_SCALE = 0.08838834764831843 * math.log2(math.e)
NEAR_FIRST = (1, 3, 2)
F32 = jnp.float32
BF16 = jnp.bfloat16


def _fold(col):
    wide = jnp.broadcast_to(col, (QB, LANES))
    lane_group = lax.broadcasted_iota(jnp.int32, (8, LANES), 1) // 16
    tile = wide[0:8]
    for j in range(1, 8):
        tile = jnp.where(lane_group == j, wide[8 * j:8 * j + 8], tile)
    return tile


def _unfold(tile):
    return jnp.concatenate(
        [jnp.broadcast_to(tile[:, 16 * j:16 * j + 1], (8, LANES)) for j in range(8)], axis=0)


def _start(copies):
    for copy in copies:
        copy.start()


def _wait(copies):
    for copy in copies:
        copy.wait()


def _attention_body(
        x_hbm, wq_hbm, k_hbm, v_hbm, wo_hbm, out_ref,
        x_f32, wq_f32, wo_f32, k_buf, v_buf, q_send, q_part, q_all, wo_bf16,
        o_send, o_part, lse_send, lse_part, o_first, ctx, acc,
        xq_sem, k_sem, v_sem, wo_sem,
        qs_ssem, qs_rsem, qg_ssem, qg_rsem, wo_ssem, wo_rsem,
        o_ssem, o_rsem, l_ssem, l_rsem, c_ssem, c_rsem):
    me = lax.axis_index("i")
    lead = me == 0
    relay = me == 2
    side = (me & 1) == 1

    def peer(j):
        return (me + j) & (N_DEV - 1)

    def remote(src, dst, ssem, rsem, j):
        return pltpu.make_async_remote_copy(
            src, dst, ssem, rsem, device_id=(peer(j),), device_id_type=pl.DeviceIdType.MESH)

    def unit_ids(u):
        h, j = u >> 2, u & (N_GROUP - 1)
        return h, j, jnp.where(h == LAST_HEAD, j, peer(j + 1))


    def head_load(hbm, buf, sem, h):
        return pltpu.make_async_copy(hbm.at[:, :, :, h], buf.at[h], sem.at[h])

    def unit_load(hbm, buf, sem, u, h, g, periods=pl.ds(0, N_PERIOD)):
        return pltpu.make_async_copy(
            hbm.at[periods, g, :, h], buf.at[h, periods, g], sem.at[u - (N_UNIT - N_KV_LOAD)])

    def wo_load(i, row0, n_rows, cols=pl.ds(0, D_MODEL)):
        rows = pl.ds(row0, n_rows)
        return pltpu.make_async_copy(wo_hbm.at[rows, cols], wo_f32.at[rows, cols], wo_sem.at[i])

    halves = [pl.ds(c * HALF, HALF) for c in range(2)]
    xq_loads = [pltpu.make_async_copy(
        wq_hbm.at[pl.ds(pl.multiple_of(me * K_SHARE, K_SHARE), K_SHARE)], wq_f32, xq_sem.at[0])]
    xq_loads += [pltpu.make_async_copy(
        x_hbm.at[0, :, pl.ds(pl.multiple_of(me * K_SHARE + LANES * t, LANES), LANES)],
        x_f32.at[:, pl.ds(LANES * t, LANES)], xq_sem.at[1 + t]) for t in range(2)]
    lead_loads = [wo_load(i, h * D_HEAD, D_HEAD) for i, h in enumerate((LEAD_HEAD, LAST_HEAD))]
    mid_loads = [wo_load(2 + i, h * D_HEAD, D_HEAD) for i, h in enumerate(MID_HEADS)]
    end_loads = [wo_load(4 + c, END_HEAD * D_HEAD, D_HEAD, halves[c]) for c in range(2)]
    side_loads = [(d, wo_load(0, first * PIECE, n * PIECE)) for d, first, n in SIDE_SHARES]
    last_k_load = unit_load(k_hbm, k_buf, k_sem, LAST_UNIT, LAST_HEAD, N_GROUP - 1)
    last_v_loads = [
        unit_load(v_hbm, v_buf, v_sem, LAST_UNIT + i, LAST_HEAD, N_GROUP - 1,
                  pl.ds(i * N_PERIOD // 2, N_PERIOD // 2)) for i in range(2)]

    _start(xq_loads)
    barrier = pltpu.get_barrier_semaphore()
    for j in reversed(NEAR_FIRST):
        pl.semaphore_signal(barrier, inc=1, device_id=(peer(j),),
                            device_id_type=pl.DeviceIdType.MESH)
    pl.when(lead)(functools.partial(_start, lead_loads + mid_loads))
    for d, load in side_loads:
        pl.when(me == d)(load.start)

    @pl.loop(0, BULK_HEADS)
    def _(h):
        head_load(k_hbm, k_buf, k_sem, h).start()
        head_load(v_hbm, v_buf, v_sem, h).start()


    own_count = jnp.where(lead, LEAD_PIECES, 0)
    for d, _, n in SIDE_SHARES:
        own_count = jnp.where(me == d, n, own_count)

    def lead_piece(i):
        skipped = (LAST_HEAD - LEAD_HEAD - 1) * HEAD_PIECES
        return LEAD_HEAD * HEAD_PIECES + i + jnp.where(i >= HEAD_PIECES, skipped, 0)

    def own_piece(i):
        p = lead_piece(i)
        for d, first, _ in SIDE_SHARES:
            p = jnp.where(me == d, first + i, p)
        return p

    def piece_copy(p, i, j):
        return remote(wo_bf16.at[p], wo_bf16.at[p], wo_ssem.at[i, j // 2], wo_rsem.at[p], j)

    def round_pieces(lo, hi):
        @pl.loop(lo, hi)
        def _(i):
            p = own_piece(i)
            w = wo_f32[pl.ds(pl.multiple_of(p * PIECE, PIECE), PIECE), :].astype(BF16)
            for t in range(N_TILE):
                wo_bf16[p, t] = w[:, LANES * t:LANES * (t + 1)]

    def share_step(i):
        @pl.when(i < own_count)
        def _():
            for j in (1, 3):
                piece_copy(own_piece(i), i, j).start()

        for d, first, n in SIDE_SHARES:
            @pl.when(relay & (i >= RELAY_LAG) & (i < RELAY_LAG + n))
            def _():
                copy = piece_copy(first + i - RELAY_LAG, i - RELAY_LAG, d)
                copy.wait_recv()
                copy.start()

    def wait_side_pieces():
        for d, first, n in SIDE_SHARES:
            @pl.loop(0, n)
            def _(i):
                copy = piece_copy(first + i, i, d)
                pl.when(relay)(copy.wait_send)
                pl.when(lead | (me == N_DEV - d))(copy.wait_recv)

    def wait_remaining_pieces():
        @pl.loop(0, own_count)
        def _(i):
            for j in (1, 3):
                piece_copy(own_piece(i), i, j).wait_send()

        @pl.loop(0, jnp.where(side, LEAD_PIECES, 0))
        def _(i):
            piece_copy(lead_piece(i), i, 1).wait_recv()

    def shared_wo(h0, n_heads, t0=0, n_tiles=N_TILE):
        w = wo_bf16[h0 * HEAD_PIECES:(h0 + n_heads) * HEAD_PIECES, pl.ds(t0, n_tiles)]
        return jnp.concatenate(
            [w[:, t].reshape(n_heads * D_HEAD, LANES) for t in range(n_tiles)], axis=1)

    def local_wo(h, cols=pl.ds(0, D_MODEL)):
        return wo_f32[pl.ds(h * D_HEAD, D_HEAD), cols].astype(BF16)


    def q_scatter(s, j):
        return remote(q_send.at[j, s], q_part.at[j - 1, s],
                      qs_ssem.at[s, j - 1], qs_rsem.at[s, j - 1], j)

    def q_gather(s, j, owner):
        block = q_all.at[owner, s]
        return remote(block, block, qg_ssem.at[s, j - 1], qg_rsem.at[s, j - 1], j)

    def ctx_gather(h, j, owner):
        block = ctx.at[h, owner]
        return remote(block, block, c_ssem.at[h, j - 1], c_rsem.at[h, j - 1], j)

    def wait_gather(gather, i):
        for j in NEAR_FIRST:
            gather(i, j, me).wait_send()
            gather(i, j, peer(N_DEV - j)).wait_recv()

    _wait(xq_loads)

    @pl.loop(0, N_DEV)
    def _(j):
        rows = pl.ds(pl.multiple_of(peer(j) * QB, QB), QB)
        q = jnp.dot(x_f32[rows, :].astype(BF16), wq_f32[...].astype(BF16),
                    preferred_element_type=F32)
        q = (q * SCORE_SCALE).astype(BF16)
        for h in range(N_HEAD):
            q_send[j, h // 2, h % 2] = q[:, h * D_HEAD:(h + 1) * D_HEAD]

    pl.semaphore_wait(barrier, N_PEER)

    @pl.loop(0, N_HEAD // 2)
    def _(s):
        _start(q_scatter(s, j) for j in NEAR_FIRST)

    pl.when(lead)(functools.partial(_wait, lead_loads))
    for d, load in side_loads:
        pl.when(me == d)(load.wait)
    round_pieces(0, own_count)

    @pl.loop(0, N_HEAD // 2)
    def _(s):
        _wait(q_scatter(s, j) for j in NEAR_FIRST)
        q = q_send[0, s].astype(F32)
        for j in NEAR_FIRST:
            q = q + q_part[j - 1, s].astype(F32)
        q_all[me, s] = q.astype(BF16)
        _start(q_gather(s, j, me) for j in NEAR_FIRST)


    def local_softmax(u, h, g):
        k = k_buf[h, :, g].reshape(N_PERIOD * QB, D_HEAD).astype(BF16)
        s = lax.dot_general(q_all[g, h >> 1, h & 1], k, (((1,), (1,)), ((), ())),
                            preferred_element_type=F32)
        m = jnp.max(s, axis=1, keepdims=True)
        p = jnp.exp2(s - m)
        total = jnp.sum(p, axis=1, keepdims=True)
        lse_send[u] = _fold(m) + jnp.log2(_fold(total))
        return p.astype(BF16), 1.0 / total

    def weighted_values(p, h, g, lo=0, hi=N_PERIOD):
        v = v_buf[h, lo:hi, g].reshape((hi - lo) * QB, D_HEAD).astype(BF16)
        return jnp.dot(p[:, lo * QB:hi * QB], v, preferred_element_type=F32)

    def partial_copy(send, part, ssem, rsem, u, slot, j):
        return remote(send.at[u], part.at[slot, j - 1],
                      ssem.at[slot, j - 1], rsem.at[slot, j - 1], j)

    lse_copy = functools.partial(partial_copy, lse_send, lse_part, l_ssem, l_rsem)
    o_copy = functools.partial(partial_copy, o_send, o_part, o_ssem, o_rsem)

    def merge_weights(u, slot):
        lses = [lse_send[u]] + [lse_part[slot, i] for i in range(N_PEER)]
        top = functools.reduce(jnp.maximum, lses)
        masses = [jnp.exp2(lse - top) for lse in lses]
        inv = 1.0 / functools.reduce(jnp.add, masses)
        return [_unfold(mass * inv) for mass in masses]

    def merge(*units):
        for u, slot in units:
            _wait(copy(u, slot, j) for j in NEAR_FIRST for copy in (lse_copy, o_copy))
        merged = []
        for u, slot in units:
            weights = merge_weights(u, slot)
            total = weights[0] * o_send[u].astype(F32)
            for j in NEAR_FIRST:
                total = total + weights[j] * o_part[slot, j - 1].astype(F32)
            merged.append(total.astype(BF16))
        return jnp.concatenate(merged, axis=0)

    def last_head_unit(g):
        return N_GROUP * LAST_HEAD + g, LAST_HEAD + g


    def project(heads, w):
        lhs = jnp.concatenate([ctx[h].reshape(SQ, D_HEAD) for h in heads], axis=1)
        return jnp.dot(lhs, w, preferred_element_type=F32)

    def project_last_head(c):
        return jnp.dot(c, shared_wo(LAST_HEAD, 1), preferred_element_type=F32)

    def accumulate_head(h, groups=()):
        wait_gather(ctx_gather, h)
        if h in MID_HEADS:
            mid_loads[MID_HEADS.index(h)].wait()
        c = merge(*map(last_head_unit, groups)) if groups else None
        acc[...] += project([h], local_wo(h) if h in MID_HEADS else shared_wo(h, 1))
        if groups:
            acc[groups[0] * QB:(groups[-1] + 1) * QB, :] += project_last_head(c)

    lead_first = (jnp.where(side, N_DEV - me, 2), jnp.where(side, 2, 1), jnp.where(side, me, 3))

    @pl.loop(0, LAST_UNIT)
    def _(u):
        h, j, g = unit_ids(u)
        last_head = h == LAST_HEAD
        own_block = j == N_GROUP - 1
        ahead = u + LOOKAHEAD

        @pl.when((ahead >= N_GROUP * BULK_HEADS) & (ahead < LAST_UNIT))
        def _():
            h_ahead, _, g_ahead = unit_ids(ahead)
            unit_load(k_hbm, k_buf, k_sem, ahead, h_ahead, g_ahead).start()
            unit_load(v_hbm, v_buf, v_sem, ahead, h_ahead, g_ahead).start()

        pl.when(ahead == LAST_UNIT)(functools.partial(_start, [last_k_load] + last_v_loads))
        pl.when((ahead == LAST_UNIT + 1) & relay)(functools.partial(_start, lead_loads))
        pl.when((ahead == LAST_UNIT + 2) & (me != 0))(functools.partial(_start, mid_loads))

        @pl.when(ahead == LAST_UNIT + 3)
        def _():
            _start(end_loads)
            wait_remaining_pieces()

        @pl.when((u & (2 * N_GROUP - 1)) == 0)
        def _():
            wait_gather(q_gather, h >> 1)

        def wait_unit(hbm, buf, sem):
            pl.when((h < BULK_HEADS) & (j == 0))(head_load(hbm, buf, sem, h).wait)
            pl.when(h >= BULK_HEADS)(unit_load(hbm, buf, sem, u, h, g).wait)

        wait_unit(k_hbm, k_buf, k_sem)
        p, inv_total = local_softmax(u, h, g)
        wait_unit(v_hbm, v_buf, v_sem)
        o_send[u] = (weighted_values(p, h, g) * inv_total).astype(BF16)

        @pl.when(last_head)
        def _():
            _start(copy(u, LAST_HEAD + j, n) for n in lead_first for copy in (lse_copy, o_copy))

        @pl.when((h < LAST_HEAD) & (j < N_GROUP - 1))
        def _():
            _start(copy(u, h, j + 1) for copy in (lse_copy, o_copy))

        @pl.when(jnp.where(last_head, j == 0, (h > 0) & own_block))
        def _():
            ctx[h - 1, me] = merge((N_GROUP * h - 1, h - 1))
            _start(ctx_gather(h - 1, n, me) for n in NEAR_FIRST)

        @pl.when(((u & 1) == 1) & (u < 2 * SHARE_STEPS))
        def _():
            share_step(u >> 1)

        @pl.when(u == SIDE_HEADS_AT)
        def _():
            wait_side_pieces()

            @pl.loop(0, SIDE_HEADS)
            def _(i):
                wait_gather(ctx_gather, i)

            @pl.loop(0, 2)
            def _(c):
                w = shared_wo(0, SIDE_HEADS, c * (N_TILE // 2), N_TILE // 2)
                acc[:, pl.ds(pl.multiple_of(c * HALF, HALF), HALF)] = project(range(SIDE_HEADS), w)

        for at, head, groups in LEAD_SCHEDULE:
            pl.when(lead & (u == at))(functools.partial(accumulate_head, head, groups))

        @pl.when(lead & (u == LAST_UNIT - 1))
        def _():
            acc[QB:2 * QB, :] += project_last_head(merge(last_head_unit(1)))


    g = N_GROUP - 1
    u, slot = last_head_unit(g)
    part = QB // 2

    def last_copy(m, j):
        rows = pl.ds(m * part, part)
        return remote(o_send.at[u, rows], o_part.at[slot, j - 1, rows],
                      o_ssem.at[slot + m, j - 1], o_rsem.at[slot + m, j - 1], j)

    last_k_load.wait()
    p, inv_total = local_softmax(u, LAST_HEAD, g)
    _start(lse_copy(u, slot, j) for j in lead_first)
    last_v_loads[0].wait()
    o_first[...] = weighted_values(p, LAST_HEAD, g, 0, N_PERIOD // 2)
    last_v_loads[1].wait()
    o = o_first[...] + weighted_values(p, LAST_HEAD, g, N_PERIOD // 2, N_PERIOD)
    o = (o * inv_total).astype(BF16)
    for m in range(2):
        o_send[u, m * part:(m + 1) * part] = o[m * part:(m + 1) * part]
        last_copy(m, lead_first[0]).start()
    _start(last_copy(m, j) for j in lead_first[1:] for m in range(2))

    @pl.when(me != 0)
    def _():
        @pl.when(relay)
        def _():
            for i, load in enumerate(lead_loads):
                load.wait()
                round_pieces(i * HEAD_PIECES, (i + 1) * HEAD_PIECES)

        accumulate_head(LEAD_HEAD, (0, 1))
        for h in MID_HEADS:
            accumulate_head(h)

    wait_gather(ctx_gather, END_HEAD)
    end_loads[0].wait()
    c = merge(last_head_unit(2))
    r = acc[:, halves[0]] + project([END_HEAD], local_wo(END_HEAD, halves[0]))
    r_last = project_last_head(c)
    out_ref[0, 0:2 * QB, halves[0]] = r[0:2 * QB].astype(out_ref.dtype)
    out_ref[0, 2 * QB:TOP, halves[0]] = (r[2 * QB:TOP] + r_last[:, :HALF]).astype(out_ref.dtype)
    acc[2 * QB:TOP, halves[1]] += r_last[:, HALF:]
    acc[TOP:, halves[0]] = r[TOP:]

    _wait(lse_copy(u, slot, j) for j in NEAR_FIRST)
    end_loads[1].wait()
    weights = merge_weights(u, slot)
    r = acc[:, halves[1]] + project([END_HEAD], local_wo(END_HEAD, halves[1]))
    out_ref[0, 0:TOP, halves[1]] = r[0:TOP].astype(out_ref.dtype)
    acc[TOP:, halves[1]] = r[TOP:]

    def finish(parts):
        lo, hi = parts[0] * part, (parts[-1] + 1) * part
        total = weights[0][lo:hi] * o_send[u, lo:hi].astype(F32)
        for j in (3, 1, 2):
            for m in parts:
                last_copy(m, j).wait_recv()
            total = total + weights[j][lo:hi] * o_part[slot, j - 1, lo:hi].astype(F32)
        r = acc[TOP + lo:TOP + hi, :] + project_last_head(total.astype(BF16))
        out_ref[0, TOP + lo:TOP + hi, :] = r.astype(out_ref.dtype)

    @pl.when(me != 0)
    def _():
        finish((0, 1))

    @pl.when(lead)
    def _():
        finish((0,))
        finish((1,))

    for m in range(2):
        for j in NEAR_FIRST:
            last_copy(m, j).wait_send()


def pallas_dist_sparse_attn_strided_kvseq_b1_sq256_skv4096_hq8_dh128_kernel(
    x: jax.Array,
    Wq: jax.Array,
    K_ext: jax.Array,
    V_ext: jax.Array,
    Wo: jax.Array,
):
    kv_shape = (N_PERIOD, N_GROUP, QB, N_HEAD, D_HEAD)
    kv_buffer = pltpu.VMEM((N_HEAD, N_PERIOD, N_GROUP, QB, D_HEAD), F32)
    q_block = (N_HEAD // 2, 2, QB, D_HEAD)
    dma = pltpu.SemaphoreType.DMA
    return pl.pallas_call(
        _attention_body,
        out_shape=jax.ShapeDtypeStruct((1, SQ, D_MODEL), BF16),
        in_specs=[pl.BlockSpec(memory_space=pl.ANY)] * 5,
        out_specs=pl.BlockSpec(memory_space=pltpu.VMEM),
        scratch_shapes=[
            pltpu.VMEM((SQ, K_SHARE), F32),
            pltpu.VMEM((K_SHARE, D_MODEL), F32),
            pltpu.VMEM((D_MODEL, D_MODEL), F32),
            kv_buffer,
            kv_buffer,
            pltpu.VMEM((N_DEV, *q_block), BF16),
            pltpu.VMEM((N_PEER, *q_block), BF16),
            pltpu.VMEM((N_GROUP, *q_block), BF16),
            pltpu.VMEM((D_MODEL // PIECE, N_TILE, PIECE, LANES), BF16),
            pltpu.VMEM((N_UNIT, QB, D_HEAD), BF16),
            pltpu.VMEM((N_SLOT, N_PEER, QB, D_HEAD), BF16),
            pltpu.VMEM((N_UNIT, 8, LANES), F32),
            pltpu.VMEM((N_SLOT, N_PEER, 8, LANES), F32),
            pltpu.VMEM((QB, D_HEAD), F32),
            pltpu.VMEM((LAST_HEAD, N_GROUP, QB, D_HEAD), BF16),
            pltpu.VMEM((SQ, D_MODEL), F32),
            dma((3,)), dma((N_KV_LOAD,)), dma((N_KV_LOAD + 1,)), dma((6,)),
            dma((N_HEAD // 2, N_PEER)), dma((N_HEAD // 2, N_PEER)),
            dma((N_HEAD // 2, N_PEER)), dma((N_HEAD // 2, N_PEER)),
            dma((LEAD_PIECES, 2)), dma((D_MODEL // PIECE,)),
            dma((N_SLOT + 1, N_PEER)), dma((N_SLOT + 1, N_PEER)),
            dma((N_SLOT, N_PEER)), dma((N_SLOT, N_PEER)),
            dma((LAST_HEAD, N_PEER)), dma((LAST_HEAD, N_PEER)),
        ],
        compiler_params=pltpu.CompilerParams(
            collective_id=0,
            vmem_limit_bytes=64 * 2**20,
            disable_semaphore_checks=True,
            disable_bounds_checks=True,
        ),
    )(x, Wq, K_ext.reshape(kv_shape), V_ext.reshape(kv_shape), Wo)
```
